```python
import numpy as np

kernel_name = "dist_rmsnorm_colshard_i_m768_n512"

def setup_inputs():
    x = np.random.randn(768, 2048).astype(np.float32)
    gamma = np.random.randn(2048).astype(np.float32)
    return {"x": x, "gamma": gamma}

def reference(x: np.ndarray, gamma: np.ndarray) -> np.ndarray:
    eps = 1e-5
    rms = np.sqrt(np.mean(x * x, axis=1, keepdims=True) + eps)
    return gamma * x / rms
```

```python
import jax
import jax.numpy as jnp
from jax import lax
from jax.experimental import pallas as pl
from jax.experimental.pallas import tpu as pltpu

N_DEV = 4
EPS = 1e-5
CHUNKS = (384, 224, 96, 64)
PEERS = (2, 1, 3)


def pallas_dist_rmsnorm_colshard_i_m768_n512_kernel(x: jax.Array, gamma: jax.Array):
    m, n = x.shape
    nc = len(CHUNKS)
    offs = [sum(CHUNKS[:c]) for c in range(nc)]
    assert sum(CHUNKS) == m and n % 128 == 0
    widths = [pl.cdiv(r, 128) * 128 for r in CHUNKS]

    def body(x_hbm, g_hbm, o_ref, xv, gv, *rest):
        sbufs, rbufs = rest[:nc], rest[nc:2 * nc]
        lsem, gsem, ssem, rsem = rest[2 * nc:]
        loads = [
            pltpu.make_async_copy(x_hbm.at[pl.ds(offs[c], CHUNKS[c])],
                                  xv.at[pl.ds(offs[c], CHUNKS[c])], lsem.at[c])
            for c in range(nc)
        ]
        gload = pltpu.make_async_copy(g_hbm, gv, gsem)
        for load in loads:
            load.start()
        gload.start()
        my = lax.axis_index("i")

        def peer(d):
            return dict(device_id=(my + d) & (N_DEV - 1),
                        device_id_type=pl.DeviceIdType.LOGICAL)

        barrier = pltpu.get_barrier_semaphore()
        for d in PEERS:
            pl.semaphore_signal(barrier, inc=1, **peer(d))
        diag = (lax.broadcasted_iota(jnp.int32, (8, 128), 1)
                - lax.broadcasted_iota(jnp.int32, (8, 128), 0))
        sends = []
        for c in range(nc):
            loads[c].wait()
            for b0 in range(0, CHUNKS[c], 128):
                h = min(128, CHUNKS[c] - b0)
                xx = xv[pl.ds(offs[c] + b0, h), :]
                sq = xx * xx
                p = (sq[:, 0:128] + sq[:, 128:256]) + (sq[:, 256:384] + sq[:, 384:512])
                rs = jnp.broadcast_to(jnp.sum(p, axis=1, keepdims=True), p.shape)
                acc = jnp.zeros((8, 128), jnp.float32)
                for j in range(0, h, 8):
                    acc = jnp.where(diag == j, rs[j:j + 8], acc)
                sbufs[c][:, pl.ds(b0, 128)] = jnp.sum(acc, axis=0, keepdims=True)
            if c == 0:
                pl.semaphore_wait(barrier, N_DEV - 1)
            for d in PEERS:
                send = pltpu.make_async_remote_copy(
                    sbufs[c], rbufs[c].at[d - 1], ssem, rsem.at[c], **peer(d))
                send.start()
                sends.append(send)
        gload.wait()
        xv[...] = xv[...] * gv[...]
        for c in range(nc):
            if c == nc - 1:
                for send in sends:
                    send.wait_send()
            pltpu.make_async_copy(rbufs[c], rbufs[c], rsem.at[c]).wait()
            for b0 in range(0, CHUNKS[c], 128):
                h = min(128, CHUNKS[c] - b0)

                def ld(r, b0=b0):
                    return jnp.broadcast_to(r[:, pl.ds(b0, 128)], (8, 128))

                tot = ((ld(sbufs[c]) + ld(rbufs[c].at[1]))
                       + (ld(rbufs[c].at[0]) + ld(rbufs[c].at[2])))
                inv = lax.rsqrt(tot * (1.0 / (N_DEV * n)) + EPS)
                sc = jnp.concatenate(
                    [jnp.where(diag == j, inv, 0.0) for j in range(0, h, 8)], axis=0)
                sc = jnp.broadcast_to(jnp.sum(sc, axis=1, keepdims=True), sc.shape)
                for j in range(0, n, 128):
                    ix = (pl.ds(offs[c] + b0, h), pl.ds(j, 128))
                    o_ref[ix] = (xv[ix] * sc).astype(o_ref.dtype)

    hbm = pl.BlockSpec(memory_space=pltpu.MemorySpace.HBM)
    return pl.pallas_call(
        body,
        out_shape=jax.ShapeDtypeStruct((m, n), jnp.bfloat16),
        in_specs=[hbm, hbm],
        out_specs=pl.BlockSpec(memory_space=pltpu.VMEM),
        scratch_shapes=[pltpu.VMEM((m, n), jnp.float32), pltpu.VMEM((1, n), jnp.float32)]
        + [pltpu.VMEM((1, w), jnp.float32) for w in widths]
        + [pltpu.VMEM((N_DEV - 1, 1, w), jnp.float32) for w in widths]
        + [pltpu.SemaphoreType.DMA((nc,)), pltpu.SemaphoreType.DMA,
           pltpu.SemaphoreType.DMA, pltpu.SemaphoreType.DMA((nc,))],
        compiler_params=pltpu.CompilerParams(
            collective_id=0, disable_bounds_checks=True, disable_semaphore_checks=True),
    )(x, gamma.reshape(1, n))
```

```python
import jax
import jax.numpy as jnp
from jax import lax
from jax.experimental import pallas as pl
from jax.experimental.pallas import tpu as pltpu

N_DEV = 4
EPS = 1e-5
LANES = 128
SUBLANES = 8

HEAD = (256, 256)
TAIL = (128, 80, 48)

FAR = 2
NEAR = (1, 3)


def pallas_dist_rmsnorm_colshard_i_m768_n512_kernel(
    x: jax.Array,
    gamma: jax.Array,
):
    m, n = x.shape
    chunks = HEAD + TAIL
    starts = [sum(chunks[:c]) for c in range(len(chunks))]
    tail_start = sum(HEAD)
    assert sum(chunks) == m and n == 4 * LANES
    inv_cols = 1.0 / (N_DEV * n)

    def kernel_body(x_hbm, gamma_hbm, out_ref, x_buf, gamma_buf, near_buf,
                    head_send, head_recv, tail_send, near_recv, far_recv,
                    load_sems, gamma_sem, send_sems, recv_sems, near_sem):
        loads = [
            pltpu.make_async_copy(
                x_hbm.at[pl.ds(r0, rows)], x_buf.at[pl.ds(r0, rows)], load_sems.at[c])
            for c, (r0, rows) in enumerate(zip(starts, chunks))
        ]
        gamma_load = pltpu.make_async_copy(gamma_hbm, gamma_buf, gamma_sem)
        for load in loads:
            load.start()
        gamma_load.start()

        my_pos = lax.axis_index("i")

        def peer(dist):
            return dict(device_id=(my_pos + dist) & (N_DEV - 1),
                        device_id_type=pl.DeviceIdType.LOGICAL)

        barrier = pltpu.get_barrier_semaphore()
        for dist in (FAR,) + NEAR:
            pl.semaphore_signal(barrier, inc=1, **peer(dist))

        sends = []

        def send(src, dst, recv_sem, dist):
            copy = pltpu.make_async_remote_copy(
                src, dst, send_sems.at[len(sends)], recv_sem, **peer(dist))
            copy.start()
            sends.append(copy)
            return copy

        tile = (SUBLANES, LANES)
        sublane = lax.broadcasted_iota(jnp.int32, tile, 0)
        diagonal = lax.broadcasted_iota(jnp.int32, tile, 1) - sublane

        def partial_mean_square(r0, rows):
            v = x_buf[pl.ds(r0, rows), :]
            squares = v * v
            sq = [squares[:, j:j + LANES] for j in range(0, n, LANES)]
            folded = (sq[0] + sq[1]) + (sq[2] + sq[3])
            sums = jnp.broadcast_to(
                jnp.sum(folded, axis=1, keepdims=True), folded.shape)
            packed = jnp.zeros(tile, jnp.float32)
            for j in range(0, rows, SUBLANES):
                packed = jnp.where(diagonal == j, sums[j:j + SUBLANES], packed)
            return jnp.sum(packed, axis=0, keepdims=True) * inv_cols

        def lanes_to_rows(v, rows):
            v = jnp.broadcast_to(v, tile)
            picked = jnp.concatenate(
                [jnp.where(diagonal == j, v, 0.0) for j in range(0, rows, SUBLANES)],
                axis=0)
            return jnp.broadcast_to(
                jnp.sum(picked, axis=1, keepdims=True), picked.shape)

        def scalars_to_rows(ref, j):
            v = [jnp.full(tile, ref[0, j + s]) for s in range(SUBLANES)]
            for bit in (1, 2, 4):
                v = [jnp.where((sublane & bit) == 0, v[i], v[i + 1])
                     for i in range(0, len(v), 2)]
            return v[0]

        def write_out(r0, rows, scale):
            for j in range(0, n, LANES):
                idx = (pl.ds(r0, rows), pl.ds(j, LANES))
                out_ref[idx] = (x_buf[idx] * scale).astype(out_ref.dtype)

        for c, rows in enumerate(HEAD):
            loads[c].wait()
            for b in range(0, rows, LANES):
                head_send[c][:, pl.ds(b, LANES)] = partial_mean_square(
                    starts[c] + b, LANES)
            if c == 0:
                pl.semaphore_wait(barrier, N_DEV - 1)
            for dist in (FAR,) + NEAR:
                send(head_send[c], head_recv[c].at[dist - 1], recv_sems.at[c], dist)
        far_copies = []
        for t, rows in enumerate(TAIL):
            c = len(HEAD) + t
            loads[c].wait()
            tail_send[t] = partial_mean_square(starts[c], rows)
            far_copies.append(send(tail_send.at[t], far_recv[t], recv_sems.at[c], FAR))
        for slot, dist in enumerate(NEAR):
            send(tail_send, near_recv.at[slot], near_sem, dist)

        gamma_load.wait()
        x_buf[...] = x_buf[...] * gamma_buf[...]
        for copy in sends:
            copy.wait_send()

        for c, rows in enumerate(HEAD):
            if c == len(HEAD) - 1:
                pltpu.make_async_copy(near_recv, near_recv, near_sem).wait()
                for t, tail_rows in enumerate(TAIL):
                    near = tail_send[t] + (near_recv[0, t] + near_recv[1, t]) + EPS
                    r = starts[len(HEAD) + t] - tail_start
                    near_buf[pl.ds(r, tail_rows), :] = lanes_to_rows(near, tail_rows)
            pltpu.make_async_copy(head_recv[c], head_recv[c], recv_sems.at[c]).wait()
            for b in range(0, rows, LANES):
                lanes = pl.ds(b, LANES)
                mean_square = (
                    (head_send[c][:, lanes] + head_recv[c][1, :, lanes])
                    + (head_recv[c][0, :, lanes] + head_recv[c][2, :, lanes]))
                write_out(starts[c] + b, LANES,
                          lanes_to_rows(lax.rsqrt(mean_square + EPS), LANES))
        for t, rows in enumerate(TAIL):
            r0 = starts[len(HEAD) + t]
            far_copies[t].wait_recv()
            for j in range(0, rows, 2 * SUBLANES):
                far = jnp.concatenate(
                    [scalars_to_rows(far_recv[t], j),
                     scalars_to_rows(far_recv[t], j + SUBLANES)], axis=0)
                near = near_buf[pl.ds(r0 - tail_start + j, 2 * SUBLANES), :]
                write_out(r0 + j, 2 * SUBLANES, lax.rsqrt(near + far))

    f32 = jnp.float32
    dma_sem = pltpu.SemaphoreType.DMA
    in_hbm = pl.BlockSpec(memory_space=pltpu.MemorySpace.HBM)
    return pl.pallas_call(
        kernel_body,
        out_shape=jax.ShapeDtypeStruct((m, n), jnp.bfloat16),
        in_specs=[in_hbm, in_hbm],
        out_specs=pl.BlockSpec(memory_space=pltpu.VMEM),
        scratch_shapes=[
            pltpu.VMEM((m, n), f32),
            pltpu.VMEM((1, n), f32),
            pltpu.VMEM((m - tail_start, LANES), f32),
            [pltpu.VMEM((1, rows), f32) for rows in HEAD],
            [pltpu.VMEM((N_DEV - 1, 1, rows), f32) for rows in HEAD],
            pltpu.VMEM((len(TAIL), 1, LANES), f32),
            pltpu.VMEM((len(NEAR), len(TAIL), 1, LANES), f32),
            [pltpu.SMEM((1, LANES), f32) for _ in TAIL],
            dma_sem((len(chunks),)),
            dma_sem,
            dma_sem(((N_DEV - 1) * len(HEAD) + len(TAIL) + len(NEAR),)),
            dma_sem((len(chunks),)),
            dma_sem,
        ],
        compiler_params=pltpu.CompilerParams(
            collective_id=0,
            disable_bounds_checks=True,
            disable_semaphore_checks=True,
        ),
    )(x, gamma.reshape(1, n))
```
